```python
import numpy as np

kernel_name = "dist_sparse_attn_causalblk_htp_bs_b2_sq256_skv256_hq4_dh64"

def setup_inputs():
    x = np.random.randn(8, 256, 512).astype(np.float32)
    Wq = np.random.randn(512, 1024).astype(np.float32) * 0.02
    K_ext = np.random.randn(8, 256, 16, 64).astype(np.float32)
    V_ext = np.random.randn(8, 256, 16, 64).astype(np.float32)
    Wo = np.random.randn(1024, 512).astype(np.float32) * 0.02
    return {"x": x, "Wq": Wq, "K_ext": K_ext, "V_ext": V_ext, "Wo": Wo}

def reference(x, Wq, K_ext, V_ext, Wo):
    B, Sq, Skv, Hq, Dh = 8, 256, 256, 16, 64
    Q = (x @ Wq).reshape(B, Sq, Hq, Dh)
    qb = (np.arange(Sq) // 64)[:, None]
    kb = (np.arange(Skv) // 64)[None, :]
    mask = kb <= qb
    scores = np.einsum('bihd,bjhd->bhij', Q, K_ext).astype(np.float32) * 0.125
    scores = np.where(mask[None, None, :, :], scores, -1e9)
    scores_max = scores.max(axis=-1, keepdims=True)
    w = np.exp(scores - scores_max)
    row_keep = mask.any(axis=1)
    w_sum = np.where(row_keep[None, None, :, None], w.sum(axis=-1, keepdims=True), 1.0)
    w = w / w_sum
    w = np.where(row_keep[None, None, :, None], w, 0.0)
    ctx = np.einsum('bhij,bjhd->bihd', w, V_ext).reshape(B, Sq, Hq * Dh)
    return ctx @ Wo
```

```python
import contextlib
import math

import jax
import jax.numpy as jnp
from jax import lax
from jax.experimental import pallas as pl
from jax.experimental.pallas import tpu as pltpu

F32, BF16 = jnp.float32, jnp.bfloat16
OWN, LEFT, RIGHT, DIAG = 0, 1, 2, 3
SCALE = 0.125 * math.log2(math.e)
NT = (((1,), (1,)), ((), ()))


def make(attn="T", scopes=False, first_rows=64, asym=True, out_dtype=BF16):
    scope = jax.named_scope if scopes else (lambda n: contextlib.nullcontext())

    def body(x_hbm, wq_hbm, k_hbm, v_hbm, wo_hbm, o_ref,
             xf, wqf, wof, kf, vf, xb, wq, wo, kp, vp, ctx, acc,
             lsem, ssem, rsem, ready):
        me = lax.axis_index("i")
        right = lax.rem(me + 1, 4)
        left = lax.rem(me + 3, 4)
        src = (me, left, right, lax.rem(me + 2, 4))

        def signal(sem, dev):
            pl.semaphore_signal(sem, inc=1, device_id=(dev,), device_id_type=pl.DeviceIdType.MESH)

        def rcopy(s, d, i, to_right):
            k = 0 if to_right else 1
            return pltpu.make_async_remote_copy(
                s, d, ssem.at[k], rsem.at[k, i],
                device_id=(right if to_right else left,), device_id_type=pl.DeviceIdType.MESH)

        fr = first_rows
        ld_wq0 = pltpu.make_async_copy(wq_hbm.at[pl.ds(0, fr)], wqf.at[pl.ds(0, fr)], lsem.at[0])
        ld_wq1 = pltpu.make_async_copy(wq_hbm.at[pl.ds(fr, 512 - fr)], wqf.at[pl.ds(fr, 512 - fr)], lsem.at[1])
        ld_wo = pltpu.make_async_copy(wo_hbm, wof, lsem.at[2])
        ld_x = pltpu.make_async_copy(x_hbm, xf, lsem.at[3])
        ld_k = [pltpu.make_async_copy(k_hbm.at[pl.ds(2 * me, 2), pl.ds(256 * src[s], 256)], kf.at[s], lsem.at[4 + s]) for s in range(4)]
        ld_v = [pltpu.make_async_copy(v_hbm.at[pl.ds(2 * me, 2), pl.ds(256 * src[s], 256)], vf.at[s], lsem.at[8 + s]) for s in range(4)]

        bar = pltpu.get_barrier_semaphore()
        with scope("start"):
            ld_wq0.start()
            if asym:
                @pl.when(me != 2)
                def _():
                    signal(bar, right)
                    signal(bar, left)
            else:
                signal(bar, right)
                signal(bar, left)
            ld_wq0.wait()
            ld_wq1.start()
            ld_wo.start()
            w = wqf[pl.ds(0, fr), :].astype(BF16)
            wq[OWN, 0, pl.ds(0, fr), :] = w[:, :128]
            wq[OWN, 1, pl.ds(0, fr), :] = w[:, 128:]

        def msgs(to_right):
            slot = LEFT if to_right else RIGHT
            a, b = (0, 1) if to_right else (1, 0)
            return [
                rcopy(wq.at[OWN, :, pl.ds(0, fr)], wq.at[slot, :, pl.ds(0, fr)], 0, to_right),
                rcopy(wq.at[OWN, a, pl.ds(fr, 512 - fr)], wq.at[slot, a, pl.ds(fr, 512 - fr)], 1, to_right),
                rcopy(wq.at[OWN, b, pl.ds(fr, 512 - fr)], wq.at[slot, b, pl.ds(fr, 512 - fr)], 2, to_right),
                rcopy(wq.at[slot, a], wq.at[DIAG, a], 3, to_right),
                rcopy(wo.at[OWN, :, :, pl.ds(64 * a, 64)], wo.at[slot, :, :, pl.ds(64 * a, 64)], 4, to_right),
                rcopy(wo.at[OWN, :, :, pl.ds(64 * b, 64)], wo.at[slot, :, :, pl.ds(64 * b, 64)], 5, to_right),
                rcopy(wo.at[slot, pl.ds(0, 2), :, pl.ds(64 * a, 64)], wo.at[DIAG, pl.ds(0, 2), :, pl.ds(64 * a, 64)], 6, to_right),
                rcopy(wo.at[slot, 2, :, pl.ds(64 * a, 64)], wo.at[DIAG, 2, :, pl.ds(64 * a, 64)], 7, to_right),
                rcopy(wo.at[slot, 3, 0, pl.ds(64 * a, 64)], wo.at[DIAG, 3, 0, pl.ds(64 * a, 64)], 8, to_right),
                rcopy(wo.at[slot, 3, 1, pl.ds(64 * a, 64)], wo.at[DIAG, 3, 1, pl.ds(64 * a, 64)], 9, to_right),
            ]

        R, L = msgs(True), msgs(False)

        with scope("bar"):
            if asym:
                odd = lax.rem(me, 2)
                pl.semaphore_wait(bar, 2 - odd)

                @pl.when(me == 2)
                def _():
                    signal(ready, right)
                    signal(ready, left)

                @pl.when(me != 1)
                def _():
                    R[0].start()

                @pl.when(me != 3)
                def _():
                    L[0].start()
            else:
                pl.semaphore_wait(bar, 2)
                R[0].start()
                L[0].start()

        with scope("wq1"):
            ld_x.start()
            ld_k[OWN].start()
            ld_v[OWN].start()
            ld_wq1.wait()
            w = wqf[pl.ds(fr, 512 - fr), :].astype(BF16)
            wq[OWN, 0, pl.ds(fr, 512 - fr), :] = w[:, :128]
            wq[OWN, 1, pl.ds(fr, 512 - fr), :] = w[:, 128:]
            if asym:
                @pl.when(me != 1)
                def _():
                    R[1].start()
                    R[2].start()

                @pl.when(me != 3)
                def _():
                    L[1].start()
                    L[2].start()

                @pl.when(odd == 1)
                def _():
                    pl.semaphore_wait(ready, 1)

                @pl.when(me == 1)
                def _():
                    R[0].start()
                    R[1].start()
                    R[2].start()

                @pl.when(me == 3)
                def _():
                    L[0].start()
                    L[1].start()
                    L[2].start()
            else:
                R[1].start()
                L[1].start()
                R[2].start()
                L[2].start()
            for s in (LEFT, RIGHT, DIAG):
                ld_k[s].start()
                ld_v[s].start()

        with scope("wo_x"):
            ld_wo.wait()
            w = wof[...].astype(BF16)
            for n in range(4):
                for p in range(2):
                    wo[OWN, n, p] = w[128 * p:128 * p + 128, 128 * n:128 * n + 128]
            ld_x.wait()
            xb[...] = (xf[...] * SCALE).astype(BF16)

        lane = lax.broadcasted_iota(jnp.int32, (64, 128), 1)
        lo = lane < 64

        def prep_kv(s):
            ld_k[s].wait()
            ld_v[s].wait()
            for b in range(2):
                for p in range(2):
                    kt = kf[s, b, pl.ds(128 * p, 128), :]
                    vt = vf[s, b, pl.ds(128 * p, 128), :]
                    if attn == "T":
                        kn = kt.T
                        l2 = lax.broadcasted_iota(jnp.int32, (256, 128), 1) < 64
                        ka = jnp.where(l2, kn, 0.0).astype(BF16)
                        kb = jnp.where(l2, 0.0, kn).astype(BF16)
                        kp[s, b, p, pl.ds(0, 128)] = ka[:128]
                        kp[s, b, p, pl.ds(128, 128)] = kb[:128]
                        kp[s, b, p, pl.ds(256, 128)] = ka[128:]
                        kp[s, b, p, pl.ds(384, 128)] = kb[128:]
                        ones = jnp.ones((16, 256), BF16)
                        for h in range(2):
                            vp[s, b, p, h, pl.ds(0, 64)] = vt[64 * h:64 * h + 64].astype(BF16)
                            vp[s, b, p, h, pl.ds(64, 16)] = ones
                    else:
                        for t, dst in ((kt, kp), (vt, vp)):
                            for j in range(2):
                                a = t[:64, 128 * j:128 * j + 128]
                                c = t[64:, 128 * j:128 * j + 128]
                                ar = pltpu.roll(a, 64, 1)
                                cr = pltpu.roll(c, 64, 1)
                                dst[s, b, p, 2 * j, pl.ds(0, 64)] = jnp.where(lo, a, 0.0).astype(BF16)
                                dst[s, b, p, 2 * j, pl.ds(64, 64)] = jnp.where(lo, 0.0, cr).astype(BF16)
                                dst[s, b, p, 2 * j + 1, pl.ds(0, 64)] = jnp.where(lo, ar, 0.0).astype(BF16)
                                dst[s, b, p, 2 * j + 1, pl.ds(64, 64)] = jnp.where(lo, 0.0, c).astype(BF16)

        def attend(s, p):
            q = jnp.dot(xb[...], wq[s, p], preferred_element_type=F32).astype(BF16)
            for b in range(2):
                qb = q[256 * b:256 * b + 256]
                if attn == "T":
                    for j in range(2):
                        nk = 128 * (j + 1)
                        st = lax.dot_general(kp[s, b, p, pl.ds(0, 2 * nk)], qb[128 * j:128 * j + 128], NT, preferred_element_type=F32)
                        outs = []
                        for h in range(2):
                            parts = [st[256 * t + 128 * h:256 * t + 128 * h + 128] for t in range(j + 1)]
                            last = parts[-1]
                            parts[-1] = jnp.concatenate([last[:64], jnp.where(lo, -jnp.inf, last[64:])], axis=0)
                            sh = jnp.concatenate(parts, axis=0) if j else parts[0]
                            m = jnp.max(sh, axis=0, keepdims=True)
                            e = jnp.exp2(sh - m).astype(BF16)
                            r = jnp.dot(vp[s, b, p, h, :, pl.ds(0, nk)], e, preferred_element_type=F32)
                            inv = 1.0 / r[64:72]
                            outs.append(r[:64] * jnp.concatenate([inv] * 8, axis=0))
                        ct = jnp.concatenate(outs, axis=0)
                        ctx[s, p, pl.ds(256 * b + 128 * j, 128)] = ct.T.astype(BF16)
                else:
                    ss = [jnp.dot(qb[64 * kb:], kp[s, b, p, kb], preferred_element_type=F32) for kb in range(4)]
                    ms = []
                    for r in range(4):
                        m = ss[0][64 * r:64 * r + 64]
                        for kb in range(1, r + 1):
                            m = jnp.maximum(m, ss[kb][64 * (r - kb):64 * (r - kb) + 64])
                        ma = jnp.max(jnp.where(lo, m, -jnp.inf), axis=1, keepdims=True)
                        mb = jnp.max(jnp.where(lo, -jnp.inf, m), axis=1, keepdims=True)
                        ms.append(jnp.where(lo, ma, mb))
                    mall = jnp.concatenate(ms, axis=0)
                    es = [jnp.exp2(ss[kb] - mall[64 * kb:]) for kb in range(4)]
                    rs = [lax.dot_general(es[kb].astype(BF16), vp[s, b, p, kb], NT, preferred_element_type=F32) for kb in range(4)]
                    for r in range(4):
                        l = es[0][64 * r:64 * r + 64]
                        c = rs[0][64 * r:64 * r + 64]
                        for kb in range(1, r + 1):
                            l = l + es[kb][64 * (r - kb):64 * (r - kb) + 64]
                            c = c + rs[kb][64 * (r - kb):64 * (r - kb) + 64]
                        la = jnp.sum(jnp.where(lo, l, 0.0), axis=1, keepdims=True)
                        lb = jnp.sum(jnp.where(lo, 0.0, l), axis=1, keepdims=True)
                        ctx[s, p, pl.ds(256 * b + 64 * r, 64)] = (c / jnp.where(lo, la, lb)).astype(BF16)

        def proj(srcs, n, pairs=(0, 1)):
            r = None
            for s in srcs:
                for p in pairs:
                    t = jnp.dot(ctx[s, p], wo[s, n, p], preferred_element_type=F32)
                    r = t if r is None else r + t
            return r

        with scope("kv_own"):
            prep_kv(OWN)
        with scope("att_own0"):
            attend(OWN, 0)
        with scope("w1"):
            R[0].wait_recv()
            L[0].wait_recv()
            R[1].wait_recv()
            L[1].wait_recv()
            for i in (3, 4, 5):
                R[i].start()
                L[i].start()
        with scope("att_own1"):
            attend(OWN, 1)
        with scope("kv_lr"):
            prep_kv(LEFT)
            prep_kv(RIGHT)
        with scope("att_1"):
            attend(LEFT, 0)
            attend(RIGHT, 1)
        with scope("w2"):
            R[2].wait_recv()
            L[2].wait_recv()
        with scope("att_2"):
            attend(LEFT, 1)
            attend(RIGHT, 0)
        with scope("kv_d"):
            prep_kv(DIAG)
        with scope("w3"):
            R[3].wait_recv()
            L[3].wait_recv()
        with scope("att_3"):
            attend(DIAG, 0)
            attend(DIAG, 1)
        with scope("w4"):
            R[4].wait_recv()
            L[4].wait_recv()
            for i in (6, 7, 8, 9):
                R[i].start()
                L[i].start()
        with scope("proj_own"):
            for n in range(4):
                acc[:, pl.ds(128 * n, 128)] = proj([OWN], n)
        with scope("w5"):
            R[5].wait_recv()
            L[5].wait_recv()
        with scope("proj_lr"):
            for n in range(4):
                acc[:, pl.ds(128 * n, 128)] += proj([LEFT, RIGHT], n)
        with scope("w6"):
            R[6].wait_recv()
            L[6].wait_recv()
        with scope("p6"):
            for n in range(2):
                o_ref[:, pl.ds(128 * n, 128)] = (acc[:, pl.ds(128 * n, 128)] + proj([DIAG], n)).astype(out_dtype)
        with scope("w7"):
            R[7].wait_recv()
            L[7].wait_recv()
        with scope("p7"):
            o_ref[:, pl.ds(256, 128)] = (acc[:, pl.ds(256, 128)] + proj([DIAG], 2)).astype(out_dtype)
        with scope("w8"):
            R[8].wait_recv()
            L[8].wait_recv()
        with scope("p8"):
            acc[:, pl.ds(384, 128)] += proj([DIAG], 3, (0,))
        with scope("w9"):
            for c in R + L:
                c.wait_send()
            R[9].wait_recv()
            L[9].wait_recv()
        with scope("p9"):
            o_ref[:, pl.ds(384, 128)] = (acc[:, pl.ds(384, 128)] + proj([DIAG], 3, (1,))).astype(out_dtype)

    def fn(x, Wq, K, V, Wo):
        Kt = jnp.transpose(K, (0, 2, 3, 1)).reshape(8, 1024, 256)
        Vt = jnp.transpose(V, (0, 2, 3, 1)).reshape(8, 1024, 256)
        any_ = pl.BlockSpec(memory_space=pl.ANY)
        if attn == "T":
            kp = pltpu.VMEM((4, 2, 2, 512, 128), BF16)
            vp = pltpu.VMEM((4, 2, 2, 2, 80, 256), BF16)
        else:
            kp = pltpu.VMEM((4, 2, 2, 4, 128, 128), BF16)
            vp = pltpu.VMEM((4, 2, 2, 4, 128, 128), BF16)
        out = pl.pallas_call(
            body,
            out_shape=jax.ShapeDtypeStruct((512, 512), out_dtype),
            in_specs=[any_] * 5,
            out_specs=pl.BlockSpec(memory_space=pltpu.VMEM),
            scratch_shapes=[
                pltpu.VMEM((512, 512), F32), pltpu.VMEM((512, 256), F32), pltpu.VMEM((256, 512), F32),
                pltpu.VMEM((4, 2, 256, 256), F32), pltpu.VMEM((4, 2, 256, 256), F32),
                pltpu.VMEM((512, 512), BF16),
                pltpu.VMEM((4, 2, 512, 128), BF16), pltpu.VMEM((4, 4, 2, 128, 128), BF16),
                kp, vp,
                pltpu.VMEM((4, 2, 512, 128), BF16), pltpu.VMEM((512, 512), F32),
                pltpu.SemaphoreType.DMA((12,)), pltpu.SemaphoreType.DMA((2,)), pltpu.SemaphoreType.DMA((2, 10)),
                pltpu.SemaphoreType.REGULAR,
            ],
            compiler_params=pltpu.CompilerParams(
                collective_id=0, vmem_limit_bytes=64 * 1024 * 1024,
                disable_bounds_checks=True, disable_semaphore_checks=True),
        )(x.reshape(512, 512), Wq, Kt, Vt, Wo)
        return out.reshape(2, 256, 512)

    return fn


_fn = make(attn="N")


def pallas_dist_sparse_attn_causalblk_htp_bs_b2_sq256_skv256_hq4_dh64_kernel(x, Wq, K_ext, V_ext, Wo):
    return _fn(x, Wq, K_ext, V_ext, Wo)
```

```python
import contextlib
import math

import jax
import jax.numpy as jnp
from jax import lax
from jax.experimental import pallas as pl
from jax.experimental.pallas import tpu as pltpu

F32, BF16, I32 = jnp.float32, jnp.bfloat16, jnp.int32
OWN, LEFT, RIGHT, DIAG = 0, 1, 2, 3
Q, O = 0, 1
SCALE = 0.125 * math.log2(math.e)
NT = (((1,), (1,)), ((), ()))
TOP, LOW = 0x78007800, 0x07800780


def words(v):
    return pltpu.bitcast(v.astype(BF16), I32)


def halves(w):
    return pltpu.bitcast(w, BF16)


def srl(v, n):
    return lax.shift_right_logical(v, jnp.full(v.shape, n, I32))


def wo_group(n, p, h):
    return (p, 2 * n + h) if n < 3 else (h, 6 + p)


def make(pack=True, scopes=False, first=(1, 3), out_dtype=BF16):
    scope = jax.named_scope if scopes else (lambda n: contextlib.nullcontext())
    GW = 24 if pack else 32
    HW = 8 if pack else 0
    HALF = 8 * GW
    B0 = HALF + HW

    def body(x_hbm, wq_hbm, k_hbm, v_hbm, wo_hbm, o_ref,
             xf, wqf, wof, kf, vf, xw, raw, wire, ctx, acc,
             lsem, ssem, rsem, fsem, ready):
        me = lax.axis_index("i")
        right = lax.rem(me + 1, 4)
        left = lax.rem(me + 3, 4)
        odd = lax.rem(me, 2)
        src = (me, left, right, lax.rem(me + 2, 4))

        def signal(sem, dev):
            pl.semaphore_signal(sem, inc=1, device_id=(dev,), device_id_type=pl.DeviceIdType.MESH)

        def remote(s, d, ss, rs, to_right):
            return pltpu.make_async_remote_copy(
                s, d, ss, rs, device_id=(right if to_right else left,), device_id_type=pl.DeviceIdType.MESH)

        cuts = (0,) + tuple(first) + (8,)
        nq = len(cuts) - 1
        ld_wq = [pltpu.make_async_copy(wq_hbm.at[pl.ds(64 * a, 64 * (b - a))], wqf.at[pl.ds(64 * a, 64 * (b - a))], lsem.at[i])
                 for i, (a, b) in enumerate(zip(cuts, cuts[1:]))]
        ld_wo = pltpu.make_async_copy(wo_hbm, wof, lsem.at[nq])
        ld_x = pltpu.make_async_copy(x_hbm, xf, lsem.at[nq + 1])
        rounds = (((OWN, 0), (OWN, 1)), ((LEFT, 0), (RIGHT, 1)), ((LEFT, 1), (RIGHT, 0)), ((DIAG, 0), (DIAG, 1)))
        ld_kv = [[pltpu.make_async_copy(h.at[pl.ds(2 * me, 2), pl.ds(256 * src[s] + 128 * p, 128)], f.at[r, i], lsem.at[nq + 2 + r])
                  for h, f in ((k_hbm, kf), (v_hbm, vf)) for i, (s, p) in enumerate(rounds[r])] for r in range(4)]

        def link(to_right):
            k, slot = (0, LEFT) if to_right else (1, RIGHT)
            a0, b0 = (0, B0) if to_right else (B0, 0)
            table = {}

            def add(name, s, d, m, row, n):
                table[name] = remote(wire.at[s, m, pl.ds(row, n)], wire.at[d, m, pl.ds(row, n)],
                                     ssem.at[k], rsem.at[k, len(table)], to_right)

            for i, (a, b) in enumerate(zip(cuts, cuts[1:])):
                add(f"qa{i}", OWN, slot, Q, a0 + GW * a, GW * (b - a))
            if pack:
                add("qh", OWN, slot, Q, HALF, HW)
            add("qb", OWN, slot, Q, b0, HALF)
            add("oa", OWN, slot, O, 0 if to_right else HALF, HALF + HW)
            add("fq", slot, DIAG, Q, a0, HALF + HW if to_right else HALF)
            add("ob", OWN, slot, O, b0, HALF)
            add("f0", slot, DIAG, O, 0 if to_right else HALF, 4 * GW + (0 if to_right else HW))
            add("f1", slot, DIAG, O, a0 + 4 * GW, 2 * GW)
            add("f2", slot, DIAG, O, a0 + 6 * GW, GW)
            add("f3", slot, DIAG, O, a0 + 7 * GW, GW)
            return table

        R, L = link(True), link(False)

        def start(*names):
            for n in names:
                R[n].start()
                L[n].start()

        def arrived(*names):
            for n in names:
                R[n].wait_recv()
                L[n].wait_recv()

        def put(m, half, g, w):
            row = half * B0 + GW * g
            if not pack:
                wire[OWN, m, pl.ds(row, 32)] = w
                return
            raw[OWN, m, pl.ds(256 * half + 32 * g, 32)] = w
            a, b, c, d = (w[8 * i:8 * i + 8] for i in range(4))
            wire[OWN, m, pl.ds(row, 8)] = (a & ~TOP) | ((d << 11) & TOP)
            wire[OWN, m, pl.ds(row + 8, 8)] = (b & ~TOP) | ((d << 7) & TOP)
            wire[OWN, m, pl.ds(row + 16, 8)] = (c & ~TOP) | ((d << 3) & 0x38003800) | (srl(d, 1) & 0x40004000)

        def put_header(m):
            ws = [raw[OWN, m, pl.ds(8 * i, 8)] for i in range(64)]
            hi = lo = jnp.zeros((8, 128), F32)
            for w in ws:
                hi = jnp.maximum(hi, pltpu.bitcast(w & 0x7F800000, F32))
                lo = jnp.maximum(lo, pltpu.bitcast((w << 16) & 0x7F800000, F32))
            top = jnp.max(jnp.max(jnp.maximum(hi, lo), axis=1, keepdims=True), axis=0, keepdims=True)
            emax = jnp.maximum(srl(pltpu.bitcast(jnp.broadcast_to(top, (8, 128)), I32), 23), 15)
            base = (emax << 23) | (emax << 7)
            k1 = k2 = ws[0] & TOP
            count = jnp.zeros((8, 128), I32)
            for i, w in enumerate(ws):
                key = w & TOP
                miss = ((base - (w & LOW)) & TOP) != key
                k1, k2 = jnp.where(miss, key | i, k1), jnp.where(miss, k1, k2)
                count = jnp.where(miss, count + 1, count)
            worst = jnp.max(jnp.max(count.astype(F32), axis=1, keepdims=True), axis=0, keepdims=True)
            bad = (jnp.broadcast_to(worst, (8, 128)) > 2.0).astype(I32)
            sub = lax.broadcasted_iota(I32, (8, 128), 0)
            ebit = lax.shift_right_logical(emax, sub) & 1
            hdr = k1 | srl(k2 & TOP, 4) | ((k2 & 63) << 16) | (ebit << 6) | (bad << 15)
            wire[OWN, m, pl.ds(HALF, 8)] = hdr

        def overflowed(s, m):
            return (wire[s, m, pl.ds(HALF, 8)][0, 0] & 0x8000) != 0

        def get_header(s, m):
            if not pack or s == OWN:
                return None
            hdr = wire[s, m, pl.ds(HALF, 8)]
            sub = lax.broadcasted_iota(I32, (8, 128), 0)
            e = (srl(hdr, 6) & 1) << sub
            for sh in (4, 2, 1):
                e = e | pltpu.roll(e, sh, 0)
            return ((e << 23) | (e << 7), hdr & 63, hdr & TOP, srl(hdr, 16) & 63, (hdr << 4) & TOP, (hdr & 0x8000) != 0)

        def get(s, m, half, g, hdr):
            row = half * B0 + GW * g
            if not pack:
                return wire[s, m, pl.ds(row, 32)]
            if s == OWN:
                return raw[OWN, m, pl.ds(256 * half + 32 * g, 32)]
            base, i1, t1, i2, t2, bad = hdr
            a, b, c = (wire[s, m, pl.ds(row + 8 * i, 8)] for i in range(3))
            d = srl(a & TOP, 11) | srl(b & TOP, 7) | (srl(c, 3) & 0x07000700) | ((c & 0x40004000) << 1)
            out = []
            for j, w in enumerate((a & ~TOP, b & ~TOP, c & ~TOP, d)):
                i = 32 * half + 4 * g + j
                top = (base - (w & LOW)) & TOP
                top = jnp.where(i1 == i, t1, jnp.where(i2 == i, t2, top))
                out.append(jnp.where(bad, raw[s, m, pl.ds(8 * i, 8)], w | top))
            return jnp.concatenate(out, axis=0)

        def raw_copy(s, d, m, to_right):
            return remote(raw.at[s, m], raw.at[d, m], fsem.at[m, 0], fsem.at[m, d], to_right)

        def send_raw(m):
            if pack:
                @pl.when(overflowed(OWN, m))
                def _():
                    for c in (raw_copy(OWN, LEFT, m, True), raw_copy(OWN, RIGHT, m, False)):
                        c.start()
                        c.wait_send()

        def recv_raw(s, m):
            if pack:
                @pl.when(overflowed(s, m))
                def _():
                    raw_copy(OWN, s, m, True).wait_recv()
                    if s == LEFT:
                        c = raw_copy(LEFT, DIAG, m, True)
                        c.start()
                        c.wait_send()

        bar = pltpu.get_barrier_semaphore()

        def put_wq(i):
            ld_wq[i].wait()
            for g in range(cuts[i], cuts[i + 1]):
                for p in range(2):
                    put(Q, p, g, words(wqf[pl.ds(64 * g, 64), pl.ds(128 * p, 128)]))

        def early(name):
            @pl.when(me == 1)
            def _():
                L[name].start()

            @pl.when(me == 3)
            def _():
                R[name].start()

        with scope("s0"):
            ld_wq[0].start()

            @pl.when(me != 2)
            def _():
                signal(bar, right)
                signal(bar, left)

            @pl.when(me != 0)
            def _():
                pl.semaphore_wait(bar, 2 - odd)

            @pl.when(me == 2)
            def _():
                signal(ready, right)
                signal(ready, left)

            for c in ld_wq[1:]:
                c.start()
        for i in range(nq):
            with scope(f"q{i}"):
                put_wq(i)
                early(f"qa{i}")

                @pl.when(me == 2)
                def _():
                    start(f"qa{i}")

                if i == 0:
                    ld_wo.start()
                    ld_x.start()
                    for r in range(4):
                        for c in ld_kv[r]:
                            c.start()
        with scope("qh"):
            if pack:
                put_header(Q)
        with scope("bar"):
            @pl.when(me == 0)
            def _():
                pl.semaphore_wait(bar, 2)

            @pl.when(odd == 1)
            def _():
                pl.semaphore_wait(ready, 1)

            @pl.when(me <= 1)
            def _():
                for i in range(nq):
                    R[f"qa{i}"].start()

            @pl.when((me == 0) | (me == 3))
            def _():
                for i in range(nq):
                    L[f"qa{i}"].start()

            if pack:
                start("qh")
            start("qb")
        with scope("wo"):
            ld_wo.wait()
            for n in range(4):
                for p in range(2):
                    for h in range(2):
                        put(O, *wo_group(n, p, h), words(wof[pl.ds(128 * p + 64 * h, 64), pl.ds(128 * n, 128)]))
            if pack:
                put_header(O)
            start("oa")
            send_raw(Q)
            send_raw(O)
        with scope("x"):
            ld_x.wait()
            xw[...] = words(xf[...] * SCALE)

        def tiles(ref):
            lo = lax.broadcasted_iota(I32, (32, 128), 1) < 64
            out = []
            for j in range(2):
                t = words(ref[:, pl.ds(128 * j, 128)])
                a, c = t[:32], pltpu.roll(t[32:], 64, 1)
                out.append(halves(jnp.concatenate([jnp.where(lo, a, 0), jnp.where(lo, 0, c)], axis=0)))
                out.append(halves(jnp.concatenate([jnp.where(lo, 0, a), jnp.where(lo, c, 0)], axis=0)))
            return out

        def per_head(xs, op, across, ident):
            lo = lax.broadcasted_iota(I32, (64, 128), 1) < 64
            even, swapped = [], []
            for r in range(4):
                blk = [xs[kb][64 * (r - kb):64 * (r - kb) + 64] for kb in range(r + 1)]
                e = blk[0] if r < 2 else op(blk[0], blk[2])
                o = ident if r == 0 else blk[1] if r < 3 else op(blk[1], blk[3])
                a = across(jnp.where(lo, e, o), axis=1, keepdims=True)
                c = across(jnp.where(lo, o, e), axis=1, keepdims=True)
                even.append(jnp.where(lo, a, c))
                swapped.append(jnp.where(lo, c, a))
            return even, swapped

        def attend(r):
            for c in ld_kv[r]:
                c.wait()
            ws = []
            for s, p in rounds[r]:
                hdr = get_header(s, Q)
                ws.append(halves(jnp.concatenate([get(s, Q, p, g, hdr) for g in range(8)], axis=0)))
            st = [None] * 4
            for step, u in ("Q0", "Q1", "S0", "Q2", "S1", "E0", "Q3", "S2", "E1", "P0", "S3", "E2", "P1", "E3", "P2", "P3"):
                u = int(u)
                i, b = divmod(u, 2)
                if step == "Q":
                    st[u] = jnp.dot(halves(xw[pl.ds(128 * b, 128), :]), ws[i], preferred_element_type=F32).astype(BF16)
                elif step == "S":
                    kt = tiles(kf.at[r, i, b])
                    st[u] = [jnp.dot(st[u][64 * kb:], kt[kb], preferred_element_type=F32) for kb in range(4)]
                elif step == "E":
                    mx = per_head(st[u], jnp.maximum, jnp.max, -jnp.inf)
                    es = [jnp.exp2(st[u][kb] - jnp.concatenate(mx[kb % 2][kb:], axis=0)) for kb in range(4)]
                    st[u] = (es, per_head(es, jnp.add, jnp.sum, 0.0)[0])
                else:
                    es, l = st[u]
                    vt = tiles(vf.at[r, i, b])
                    rs = [lax.dot_general(es[kb].astype(BF16), vt[kb], NT, preferred_element_type=F32) for kb in range(4)]
                    s, p = rounds[r][i]
                    for q in range(4):
                        c = rs[0][64 * q:64 * q + 64]
                        for kb in range(1, q + 1):
                            c = c + rs[kb][64 * (q - kb):64 * (q - kb) + 64]
                        inv = pltpu.reciprocal(l[q], approx=True)
                        inv = inv * (2.0 - l[q] * inv)
                        ctx[s, p, pl.ds(128 * b + 32 * q, 32)] = words(c * inv)

        def project(work, first=False, last=False):
            hdrs = {s: get_header(s, O) for s in sorted({s for v in work.values() for s, _ in v})}
            ntiles = sum(len(v) for v in work.values())
            split = 4 // math.gcd(ntiles, 4)
            rows = 512 // split
            for n, terms in work.items():
                wt = [halves(jnp.concatenate([get(s, O, *wo_group(n, p, h), hdrs[s]) for h in range(2)], axis=0)) for s, p in terms]
                for j in range(split):
                    r = None if first else acc[n, pl.ds(rows * j, rows)]
                    for (s, p), w in zip(terms, wt):
                        t = jnp.dot(halves(ctx[s, p, pl.ds(rows // 2 * j, rows // 2)]), w, preferred_element_type=F32)
                        r = t if r is None else r + t
                    if last:
                        o_ref[pl.ds(rows * j, rows), pl.ds(128 * n, 128)] = r.astype(out_dtype)
                    else:
                        acc[n, pl.ds(rows * j, rows)] = r

        with scope("att0"):
            attend(0)
        with scope("w1"):
            arrived(*[f"qa{i}" for i in range(nq)])
            if pack:
                arrived("qh")
            start("fq", "ob")
            recv_raw(LEFT, Q)
            recv_raw(RIGHT, Q)
        with scope("att1"):
            attend(1)
        with scope("w2"):
            arrived("qb")
        with scope("att2"):
            attend(2)
        with scope("p_own"):
            project({n: [(OWN, 0), (OWN, 1)] for n in range(4)}, first=True)
        with scope("w3"):
            arrived("oa")
            start("f0", "f1", "f2", "f3")
            recv_raw(LEFT, O)
            recv_raw(RIGHT, O)
        with scope("p_a"):
            project({n: [(LEFT, 0), (RIGHT, 1)] for n in range(3)})
        with scope("w4"):
            arrived("fq")
            recv_raw(DIAG, Q)
        with scope("att3"):
            attend(3)
        with scope("w5"):
            arrived("ob")
        with scope("p_b"):
            project({n: [(LEFT, 1), (RIGHT, 0)] + ([(LEFT, 0), (RIGHT, 1)] if n == 3 else []) for n in range(4)})
        with scope("w6"):
            arrived("f0")
            recv_raw(DIAG, O)
        with scope("p6"):
            project({n: [(DIAG, 0), (DIAG, 1)] for n in range(2)}, last=True)
        with scope("w7"):
            arrived("f1")
        with scope("p7"):
            project({2: [(DIAG, 0), (DIAG, 1)]}, last=True)
        with scope("w8"):
            arrived("f2")
        with scope("p8"):
            project({3: [(DIAG, 0)]})
        with scope("w9"):
            for c in list(R.values()) + list(L.values()):
                c.wait_send()
            arrived("f3")
        with scope("p9"):
            project({3: [(DIAG, 1)]}, last=True)

    def fn(x, Wq, K, V, Wo):
        Kt = jnp.transpose(K, (0, 2, 3, 1)).reshape(8, 1024, 256)
        Vt = jnp.transpose(V, (0, 2, 3, 1)).reshape(8, 1024, 256)
        any_ = pl.BlockSpec(memory_space=pl.ANY)
        out = pl.pallas_call(
            body,
            out_shape=jax.ShapeDtypeStruct((512, 512), out_dtype),
            in_specs=[any_] * 5,
            out_specs=pl.BlockSpec(memory_space=pltpu.VMEM),
            scratch_shapes=[
                pltpu.VMEM((512, 512), F32), pltpu.VMEM((512, 256), F32), pltpu.VMEM((256, 512), F32),
                pltpu.VMEM((4, 2, 2, 128, 256), F32), pltpu.VMEM((4, 2, 2, 128, 256), F32),
                pltpu.VMEM((256, 512), I32),
                pltpu.VMEM((4, 2, 512, 128), I32), pltpu.VMEM((4, 2, 2 * HALF + HW, 128), I32),
                pltpu.VMEM((4, 2, 256, 128), I32), pltpu.VMEM((4, 512, 128), F32),
                pltpu.SemaphoreType.DMA((12,)), pltpu.SemaphoreType.DMA((2,)), pltpu.SemaphoreType.DMA((2, 16)),
                pltpu.SemaphoreType.DMA((2, 4)), pltpu.SemaphoreType.REGULAR,
            ],
            compiler_params=pltpu.CompilerParams(
                collective_id=0, vmem_limit_bytes=64 * 1024 * 1024,
                disable_bounds_checks=True, disable_semaphore_checks=True),
        )(x.reshape(512, 512), Wq, Kt, Vt, Wo)
        return out.reshape(2, 256, 512)

    return fn


_fn = make(pack=True)


def pallas_dist_sparse_attn_causalblk_htp_bs_b2_sq256_skv256_hq4_dh64_kernel(x, Wq, K_ext, V_ext, Wo):
    return _fn(x, Wq, K_ext, V_ext, Wo)
```

```python
import contextlib
import math

import jax
import jax.numpy as jnp
from jax import lax
from jax.experimental import pallas as pl
from jax.experimental.pallas import tpu as pltpu

F32, BF16, I32 = jnp.float32, jnp.bfloat16, jnp.int32
OWN, LEFT, RIGHT, DIAG = range(4)
WQ, WO = range(2)
SHARD = {"o": OWN, "l": LEFT, "r": RIGHT, "d": DIAG}
PAIRS = ((OWN, 0), (OWN, 1), (LEFT, 0), (RIGHT, 1), (LEFT, 1), (RIGHT, 0), (DIAG, 0), (DIAG, 1))
TILE_ROWS = {0: (1, 4), 1: (1, 4), 2: (0, 1), 5: (2, 3), 3: (3, 4), 4: (3, 4)}
SCORE_SCALE = 0.125 * math.log2(math.e)

LOW, HIGH, ESCAPES, WIRE_TILES = (0, 29), (16, 23), 22, 45
SIGNS = -0x7FFF8000

SCHED = """
@bx s:oah,ox,oa0 x Q1 Q0
@w0 kv0
@b0 Q3 S0 Q2 S1 E1 E0 P0 P1
@w1 a:qa s:fq,fqx,oa1,obh chkQlr kv1
@b1 M2:o0 Wl0.0 M1:o0 Wl0.1 S3 Wl0.2 E3 Wl0.3 S2 Wr1.0 M3:o0 Wr1.1 E2 M0:o0 Wr1.2 P2 Q4 Wr1.3 P3 Q5
@w2 kv2 kv3
@b2 S4 Q6 S6 Q7 S5 E5 E4 E6 P4 P6 S7 P5 E7 P7
@w3 a:qb a:oah,ox s:foh,fox,ob0,ob1 chkOlr kv4 kv5
@b3 M1:o1 Wl1.0 M0:o1 Wl1.1 M2:o1 Wl1.2 Wl1.3 M3:o1 Q8 Wr0.0 Wr0.1 Wr0.2 S8 Hl0.0 Q9 Wr0.3 Q10 Hl0.1 S9 Hr1.0 Q11 Hl0.2 Hl0.3 Hr1.1 E8 S10 Hr1.2 P8 Hr1.3 S11 E9 E10 P9 E11 P10 P11
@w4 a:oa0 s:f0,f1 ifn:a:oa1+s:f2,f3 a:fq,fqx chkQd kv6 kv7
@b4 M1:l0,r1 Wd0.0 Wd0.1 M0:l0,r1 Wd0.2 Wd0.3 Q12 Wd1.0 S12 Wd1.1 Q13 Wd1.2 Wd1.3 Q14 S13 Q15 E12 S14 E13 P13 P12 E14 S15 E15 P14 P15
@w5 if0:a:oa1+s:f2,f3 a:obh
@b5 M2:l0 Hl1.0 Hl1.1 M3:l0 M2:r1 Hr0.0 M3:r1 Hr0.1 Hl1.2 Hr0.2 Hr0.3 Hl1.3
@w6 a:foh,fox,ob0 chkOd
@b6 M0:r0 M1:l1 M0:l1 Hd1.0 M1:r0 Hd0.0 Hd0.1 Hd0.2 Hd1.1 Hd1.2 Hd1.3 Hd0.3
@w7 a:ob1
@b7 M2:l1,r0 M3:l1,r0
@w8 a:f0
@b8 M0:d0,d1
@w9 a:f1
@b9 M1:d0,d1
@w10 a:f2
@b10 M2:d0,d1
@w11 sent a:f3
@b11 M3:d0,d1
"""
LINK = ""


def words(v):
    return pltpu.bitcast(v.astype(BF16), I32)


def as_bf16(w):
    return pltpu.bitcast(w, BF16)


def shift(v, n):
    if n >= 0:
        return v << n if n else v
    return lax.shift_right_logical(v, jnp.full(v.shape, -n, I32))


def reverse_bits(v):
    for n, mask in ((1, 0x55555555), (2, 0x33333333), (4, 0x0F0F0F0F), (8, 0x00FF00FF), (16, 0x0000FFFF)):
        v = (shift(v, -n) & mask) | ((v & mask) << n)
    return v


def low_bytes(w):
    return (w[:8] & 0x00FF00FF) | ((w[8:] & 0x00FF00FF) << 8)


def encode_high(ws):
    peak = jnp.zeros((8, 128), F32)
    for w in ws:
        for half in (w, w << 16):
            peak = jnp.maximum(peak, pltpu.bitcast(half & 0x7F800000, F32))
    lane_peak = jnp.broadcast_to(jnp.max(peak, axis=0, keepdims=True), (8, 128))
    lower = (peak < lane_peak).astype(I32)
    lane_top = shift(pltpu.bitcast(lane_peak, I32), -23)
    top = lane_top - lower
    top = (top << 23) | (top << 7)
    planes = [None] * 6
    marks = end = jnp.zeros((8, 128), I32)
    for i, w in enumerate(ws):
        drop = top - (w & 0x7F807F80)
        fields = [(4 + i // 16, shift(w & SIGNS, -(i % 16)))]
        for q, pos in ((shift(drop, -24), 16), (shift(drop, -8) & 0x7F, 0)):
            big = q > 2
            end = end + jnp.where(big, q - 2, 0)
            marks = marks | (1 << (end & 31))
            fields.append((i // 8, shift(jnp.where(big, 3, q), pos + 2 * (i % 8))))
        for k, f in fields:
            planes[k] = f if planes[k] is None else planes[k] | f
    return jnp.concatenate(planes, axis=0), (shift(marks, -1), end, lower, lane_top)


def merge_escapes(first, second):
    (marks0, end0, lower0, top0), (marks1, end1, lower1, top1) = first, second
    fits = end0 + end1 <= 29
    shared = (marks0 << 3) | (lower1 << 2) | (lower0 << 1) | jnp.where(fits, reverse_bits(marks1) | 1, 0)
    spill = jnp.where(fits, 0, marks1)
    count = jnp.where(fits, 0, jnp.where((end0 > 29) | (end1 > 31), 2, 1))
    for n in (4, 2, 1):
        spill = spill | pltpu.roll(spill, n, 0)
        count = count + pltpu.roll(count, n, 0)
    overflow = jnp.broadcast_to(jnp.max(count.astype(F32), axis=1, keepdims=True), (8, 128)) > 1.0
    meta = top0 | (top1 << 8) | (overflow.astype(I32) << 16)
    row = lax.broadcasted_iota(I32, (8, 128), 0)
    return shared, jnp.where(row == 0, spill, meta)[:2]


def decode_high(p, plane, shared, spill, meta):
    top = (shift(meta, -8 * p) & 0xFF) - (shift(shared, -1 - p) & 1)
    yield jnp.where((top & 1) != 0, 0, 0x00800080)
    top = ((top << 23) | (top << 7)) & 0x7F007F00
    marks = jnp.where((shared & 1) != 0, reverse_bits(shared), spill) if p else shift(shared, -3)
    end = jnp.full((8, 128), 0.5, F32)
    for i in range(32):
        if i % 8 == 0:
            code = plane(i // 8)
            big = code & shift(code, -1) & 0x55555555
            code = code - big
        w = top - (shift(code, 8 - 2 * (i % 8)) & 0x03000300)
        for pos in (16, 0):
            rest = marks & (marks + (shift(big, 31 - pos - 2 * (i % 8)) >> 31))
            new_end = jnp.maximum(end, (marks ^ rest).astype(F32))
            w = w - shift(pltpu.bitcast(new_end, I32) - pltpu.bitcast(end, I32), pos - 15)
            marks, end = rest, new_end
        yield w | (shift(plane(4 + i // 16), i % 16) & SIGNS)


def make(sched=SCHED, scopes=False, first=(3, 8), out_dtype=BF16, flags=None, shared_send=True, checks=False):
    scope = jax.named_scope if scopes else (lambda n: contextlib.nullcontext())

    def body(x_hbm, wq_hbm, k_hbm, v_hbm, wo_hbm, o_ref,
             xf, wqf, wof, kf, vf, head, xw, full, wire, trailer, ctx, acc,
             load_sem, send_sem, recv_sem, plain_sem, ready):
        me = lax.axis_index("i")
        right, left = lax.rem(me + 1, 4), lax.rem(me + 3, 4)
        owner = (me, left, right, lax.rem(me + 2, 4))
        odd = lax.rem(me, 2)

        def signal_neighbours(sem):
            for dev in (right, left):
                pl.semaphore_signal(sem, inc=1, device_id=(dev,), device_id_type=pl.DeviceIdType.MESH)

        def remote(src, dst, ssem, rsem, k):
            return pltpu.make_async_remote_copy(
                src, dst, ssem, rsem, device_id=((right, left)[k],), device_id_type=pl.DeviceIdType.MESH)

        urgent = (me == 1).astype(I32)
        cuts = (1,) + tuple(first) + (16,)
        pieces = range(len(cuts) - 1)
        loads = []

        def load(src, dst):
            loads.append(pltpu.make_async_copy(src, dst, load_sem.at[len(loads)]))
            return loads[-1]

        def load_wq(k, p, a, b):
            rows = pl.ds(32 * a, 32 * (b - a))
            return load(wq_hbm.at[rows, pl.ds(pl.multiple_of(128 * p, 128), 128)], wqf.at[k, rows])

        ld_wq = [load_wq(0, urgent, a, b) for a, b in zip(cuts, cuts[1:])] + [load_wq(0, urgent, 0, 1)]
        ld_wq2 = load_wq(1, 1 - urgent, 0, 16)
        ld_wo = load(wo_hbm, wof)
        ld_x = load(x_hbm, xf)
        ld_kv = [[load(h.at[pl.ds(2 * me, 2), pl.ds(256 * owner[s] + 128 * p, 128)], f.at[i])
                  for h, f in ((k_hbm, kf), (v_hbm, vf))] for i, (s, p) in enumerate(PAIRS)]

        def link(k):
            near, a, b = (LEFT, RIGHT)[k], k, 1 - k
            table = {}

            def add(name, src, dst):
                table[name] = remote(src, dst, send_sem.at[k, 0 if shared_send else len(table)], recv_sem.at[k, len(table)], k)

            def tiles(name, s, d, m, t, n):
                add(name, wire.at[s, m, pl.ds(8 * t, 8 * n)], wire.at[d, m, pl.ds(8 * t, 8 * n)])

            for i in pieces:
                tiles(f"qa{i}", OWN, near, WQ, LOW[a] + cuts[i], cuts[i + 1] - cuts[i])
                tiles(f"qb{i}", OWN, near, WQ, LOW[b] + cuts[i], cuts[i + 1] - cuts[i])
            tiles("qbz", OWN, near, WQ, LOW[b], 1)
            for name, m in (("q", WQ), ("o", WO)):
                tiles(name + "ah", OWN, near, m, HIGH[a] - a, 7)
                tiles(name + "bh", OWN, near, m, HIGH[b], 6)
                add(name + "x", trailer.at[OWN, m], trailer.at[near, m])
            for i in range(2):
                tiles(f"oa{i}", OWN, near, WO, LOW[a] + 8 * i, 8)
                tiles(f"ob{i}", OWN, near, WO, LOW[b] + 8 * i, 8)
            tiles("fq", near, DIAG, WQ, 23 * k, 23 - k)
            tiles("foh", near, DIAG, WO, HIGH[a] - a, 6 + k)
            add(("fqx", "fox")[k], trailer.at[near, k], trailer.at[DIAG, k])
            for n in range(4):
                tiles(f"f{n}", near, DIAG, WO, LOW[a] + 4 * n, 4)
            tiles("qaz", OWN, near, WQ, LOW[a], 1)
            add("head", wq_hbm.at[pl.ds(0, 32), pl.ds(128 * a, 128)], head.at[k])
            return table

        links = (link(0), link(1))

        def send(*names, when=(None, None)):
            for table, cond in zip(links, when):
                def start():
                    for n in names:
                        if n in table:
                            table[n].start()
                if cond is None:
                    start()
                elif cond is not False:
                    pl.when(cond)(start)

        def receive(*names):
            for table in links:
                for n in names:
                    if n in table:
                        table[n].wait_recv()

        def put_low(m, p, j, w):
            full[OWN, m, p, pl.ds(16 * j, 16)] = w
            wire[OWN, m, pl.ds(pl.multiple_of(8 * (LOW[1] * p + j), 8), 8)] = low_bytes(w)

        def put_high(m, p):
            planes, escapes = encode_high([full[OWN, m, p, pl.ds(8 * i, 8)] for i in range(32)])
            wire[OWN, m, pl.ds(pl.multiple_of(8 * (HIGH[0] + 7 * p), 8), 48)] = planes
            return escapes

        def put_escapes(m, pair0, pair1):
            shared, tail = merge_escapes(pair0, pair1)
            wire[OWN, m, pl.ds(8 * ESCAPES, 8)] = shared
            trailer[OWN, m] = tail

        def overflow_bits(*shards):
            bits = None
            for n, (s, m) in enumerate(shards):
                bit = shift(trailer[s, m, pl.ds(1, 1)] & 0x10000, n - 16)
                bits = bit if bits is None else bits | bit
            bits = bits[0, 0]
            return [(bits & (1 << n)) != 0 for n in range(len(shards))]

        def plain(s, d, m, k):
            return remote(full.at[s, m], full.at[d, m], plain_sem.at[m, 0], plain_sem.at[m, d], k)

        def send_plain(*args):
            copy = plain(*args)
            copy.start()
            copy.wait_send()

        def receive_plain(m, shards):
            for s, overflow in zip(shards, overflow_bits(*((s, m) for s in shards))):
                @pl.when(overflow)
                def _():
                    plain(OWN, s, m, 0).wait_recv()
                    if s == LEFT:
                        send_plain(LEFT, DIAG, m, 0)

        barrier = pltpu.get_barrier_semaphore()
        with scope("s0"):
            ld_wq[0].start()
            pl.when(me != 2)(lambda: signal_neighbours(barrier))
            pl.when(me != 0)(lambda: pl.semaphore_wait(barrier, 2 - odd))
            send("head", when=(me == 3, me == 1))
            pl.when(me == 2)(lambda: signal_neighbours(ready))
            for c in ld_wq[1:]:
                c.start()
        for i in pieces:
            with scope(f"q{i}"):
                ld_wq[i].wait()
                for j in range(cuts[i], cuts[i + 1]):
                    put_low(WQ, urgent, j, words(wqf[0, pl.ds(32 * j, 32)]))
                send(f"qa{i}", when=(me >= 2, me == 1))
                if i != pieces[-1]:
                    send(f"qb{i}", when=(False, me == 2))
                if i == 0:
                    for c in loads[len(ld_wq):]:
                        c.start()
        with scope("qh"):
            ld_wq[-1].wait()
            put_low(WQ, urgent, 0, words(wqf[0, pl.ds(0, 32)]))
            early = put_high(WQ, urgent)
        with scope("qq"):
            ld_wq2.wait()
            for j in range(16):
                put_low(WQ, 1 - urgent, j, words(wqf[1, pl.ds(32 * j, 32)]))
            send(*(f"qa{i}" for i in pieces), when=(False, me == 2))
            late = put_high(WQ, 1 - urgent)
            put_escapes(WQ, [jnp.where(me == 1, b, a) for a, b in zip(early, late)],
                        [jnp.where(me == 1, a, b) for a, b in zip(early, late)])
        with scope("bar"):
            pl.when(me == 0)(lambda: pl.semaphore_wait(barrier, 2))
            pl.when(odd == 1)(lambda: pl.semaphore_wait(ready, 1))
            send(*(f"qa{i}" for i in pieces), when=(me <= 1, (me == 0) | (me == 3)))
            send("qaz", when=(me != 3, me != 1))
            send("qah", "qx")
            send(*(f"qb{i}" for i in pieces[:-1]), when=(None, me != 2))
            send(f"qb{pieces[-1]}", "qbz", "qbh")
        with scope("wo"):
            ld_wo.wait()
            for p in range(2):
                for j in range(16):
                    put_low(WO, p, j, words(wof[pl.ds(128 * p + 32 * (j % 4), 32), pl.ds(128 * (j // 4), 128)]))
            put_escapes(WO, put_high(WO, 0), put_high(WO, 1))
            for m, overflow in enumerate(overflow_bits((OWN, WQ), (OWN, WO))):
                @pl.when(overflow)
                def _():
                    send_plain(OWN, LEFT, m, 0)
                    send_plain(OWN, RIGHT, m, 1)

        low_masks, decoders, pending = {}, {}, []

        def add_low(s, m, p, j, high):
            keep, borrow = low_masks[s, m, p]
            v = wire[s, m, pl.ds(8 * (LOW[p] + j), 8)]
            return [h + low - ((low & borrow) << 1) for h, low in zip(high, (v & keep, shift(v, -8) & keep))]

        def decoder(s, m, p):
            spill, meta = (jnp.broadcast_to(trailer[s, m, pl.ds(r, 1)], (8, 128)) for r in range(2))
            is_plain = (meta & 0x10000) != 0
            high = decode_high(p, lambda k: wire[s, m, pl.ds(8 * (HIGH[p] + k), 8)],
                               wire[s, m, pl.ds(8 * ESCAPES, 8)], spill, meta)
            low_masks[s, m, p] = (jnp.where(is_plain, 0, 0x00FF00FF), next(high))
            for g in range(4):
                out = [jnp.where(is_plain, full[s, m, p, pl.ds(64 * g + 8 * i, 8)], next(high)) for i in range(8)]
                if m == WQ:
                    out = [w for j in range(4) for w in add_low(s, m, p, 4 * g + j, out[2 * j:2 * j + 2])]
                full[s, m, p, pl.ds(64 * g, 64)] = jnp.concatenate(out, axis=0)
                pending.append(out[-1])
                yield

        def after_decoding(v):
            if not pending:
                return v
            first = v[:8]
            while pending:
                w = pending.pop()
                first = jnp.where(me < 0, w if v.dtype == I32 else pltpu.bitcast(w, v.dtype), first)
            return jnp.concatenate([first, v[8:]], axis=0)

        def kv_tiles(ref):
            lo = lax.broadcasted_iota(I32, (64, 128), 1) < 64
            zero = jnp.zeros((64, 128), F32)
            out = []
            for j in range(2):
                t = after_decoding(ref[:, pl.ds(128 * j, 128)])
                a, b = t[:64], t[64:]
                for u, v in ((a, zero), (zero, b), (jnp.where(lo, a, 0.0), jnp.where(lo, 0.0, pltpu.roll(b, 64, 1)))):
                    out.append(jnp.concatenate([u, v], axis=0).astype(BF16))
            return out

        def per_head(x, r, op, across, identity):
            lo = lax.broadcasted_iota(I32, (64, 128), 1) < 64
            a = [x[r, t] if t % 3 == 0 else jnp.where(lo, x[r, t], identity) for t in (0, 2, 3, 5) if (r, t) in x]
            b = [x[r, t] if t % 3 == 1 else jnp.where(lo, identity, x[r, t]) for t in (1, 2, 4, 5) if (r, t) in x]
            a, b = (across(v[0] if len(v) == 1 else op(*v), axis=1, keepdims=True) for v in (a, b))
            return a, b, jnp.where(lo, a, b)

        state = {}

        def attend(step, u):
            i, b = divmod(u, 2)
            s, p = PAIRS[i]
            if step == "Q":
                state[u] = jnp.dot(as_bf16(xw[pl.ds(128 * b, 128), :]), as_bf16(after_decoding(full[s, WQ, p])),
                                   preferred_element_type=F32)
            elif step == "S":
                q, kt, scores = state[u], kv_tiles(kf.at[i, b]), {}
                for t, (r0, r1) in TILE_ROWS.items():
                    v = jnp.dot(q[64 * r0:64 * r1].astype(BF16), kt[t], preferred_element_type=F32)
                    for r in range(r0, r1):
                        scores[r, t] = v[64 * (r - r0):64 * (r - r0 + 1)]
                state[u] = scores
            elif step == "E":
                scores, weights = state[u], {}
                for r in range(4):
                    row_max = per_head(scores, r, jnp.maximum, jnp.max, -jnp.inf)
                    for t in range(6):
                        if (r, t) in scores:
                            weights[r, t] = jnp.exp2(scores[r, t] - row_max[t % 3])
                state[u] = weights, [per_head(weights, r, jnp.add, jnp.sum, 0.0)[2] for r in range(4)]
            else:
                (weights, total), vt, out = state[u], kv_tiles(vf.at[i, b]), {}
                for t, (r0, r1) in TILE_ROWS.items():
                    w = jnp.concatenate([weights[r, t] for r in range(r0, r1)], axis=0).astype(BF16)
                    v = lax.dot_general(w, vt[t], (((1,), (1,)), ((), ())), preferred_element_type=F32)
                    for r in range(r0, r1):
                        part = v[64 * (r - r0):64 * (r - r0 + 1)]
                        out[r] = out[r] + part if r in out else part
                for r in range(4):
                    inv = pltpu.reciprocal(total[r], approx=True)
                    inv = inv * (2.0 - total[r] * inv)
                    ctx[s, p, pl.ds(128 * b + 32 * r, 32)] = words(out[r] * inv)

        terms_left = [8] * 4

        def project(n, terms):
            ws = []
            for s, p in terms:
                w = full[s, WO, p, pl.ds(64 * n, 64)]
                if s != OWN:
                    w = jnp.concatenate([t for j in range(4) for t in add_low(
                        s, WO, p, 4 * n + j, (w[16 * j:16 * j + 8], w[16 * j + 8:16 * j + 16]))], axis=0)
                ws.append(as_bf16(after_decoding(w)))
            fresh = terms_left[n] == 8
            terms_left[n] -= len(terms)
            rows = 128 * len(terms)
            for r0 in range(0, 512, rows):
                total = None if fresh else acc[n, pl.ds(r0, rows)]
                for (s, p), w in zip(terms, ws):
                    t = jnp.dot(as_bf16(ctx[s, p, pl.ds(r0 // 2, rows // 2)]), w, preferred_element_type=F32)
                    total = t if total is None else total + t
                if terms_left[n]:
                    acc[n, pl.ds(r0, rows)] = total
                else:
                    o_ref[pl.ds(r0, rows), pl.ds(128 * n, 128)] = total.astype(out_dtype)

        def do(tok):
            if tok == "x":
                ld_x.wait()
                xw[...] = words(xf[...] * SCORE_SCALE)
            elif tok == "sent":
                for table, sent_head in zip(links, (me == 3, me == 1)):
                    pl.when(sent_head)(table["head"].wait_send)
                    pl.when(~sent_head)(table["qaz"].wait_send)
                    for n, copy in table.items():
                        if n not in ("head", "qaz"):
                            copy.wait_send()
            elif tok == "a:qa":
                receive(*(f"qa{i}" for i in pieces), "qah", "qx")
                pl.when(me != 0)(lambda: receive("qaz"))

                @pl.when(me == 0)
                def _():
                    receive("head")
                    for k in range(2):
                        wire[(LEFT, RIGHT)[k], WQ, pl.ds(8 * LOW[k], 8)] = low_bytes(words(head[k]))
            elif tok == "a:qb":
                receive(*(f"qb{i}" for i in pieces), "qbz", "qbh")
            elif tok.startswith("if"):
                @pl.when((me == 0) if tok[2] == "0" else (me != 0))
                def _():
                    for t in tok[4:].split("+"):
                        do(t)
            elif tok.startswith("a:"):
                receive(*tok[2:].split(","))
            elif tok.startswith("s:"):
                send(*tok[2:].split(","))
            elif tok.startswith("kv"):
                for c in ld_kv[int(tok[2:])]:
                    c.wait()
            elif tok.startswith("chk"):
                receive_plain({"Q": WQ, "O": WO}[tok[3]], [SHARD[c] for c in tok[4:]])
            elif tok[0] in "WH":
                key = (SHARD[tok[1]], WQ if tok[0] == "W" else WO, int(tok[2]))
                next(decoders.setdefault(key, decoder(*key)))
            elif tok[0] == "M":
                project(int(tok[1]), [(SHARD[t[0]], int(t[1])) for t in tok[3:].split(",")])
            else:
                attend(tok[0], int(tok[1:]))

        for line in sched.split("@")[1:]:
            name, *toks = line.split()
            with scope(name):
                for tok in toks:
                    do(tok)
                pending.clear()
        assert terms_left == [0] * 4

    def fn(x, Wq, K, V, Wo):
        Kt = jnp.transpose(K, (0, 2, 3, 1)).reshape(8, 1024, 256)
        Vt = jnp.transpose(V, (0, 2, 3, 1)).reshape(8, 1024, 256)
        out = pl.pallas_call(
            body,
            out_shape=jax.ShapeDtypeStruct((512, 512), out_dtype),
            in_specs=[pl.BlockSpec(memory_space=pl.ANY)] * 5,
            out_specs=pl.BlockSpec(memory_space=pltpu.VMEM),
            scratch_shapes=[
                pltpu.VMEM((512, 512), F32), pltpu.VMEM((2, 512, 128), F32), pltpu.VMEM((256, 512), F32),
                pltpu.VMEM((8, 2, 128, 256), F32), pltpu.VMEM((8, 2, 128, 256), F32), pltpu.VMEM((2, 32, 128), F32),
                pltpu.VMEM((256, 512), I32),
                pltpu.VMEM((4, 2, 2, 256, 128), I32), pltpu.VMEM((4, 2, 8 * WIRE_TILES, 128), I32),
                pltpu.VMEM((4, 2, 2, 128), I32),
                pltpu.VMEM((4, 2, 256, 128), I32), pltpu.VMEM((4, 512, 128), F32),
                pltpu.SemaphoreType.DMA((24,)), pltpu.SemaphoreType.DMA((2, 28)), pltpu.SemaphoreType.DMA((2, 28)),
                pltpu.SemaphoreType.DMA((2, 4)), pltpu.SemaphoreType.REGULAR,
            ],
            compiler_params=pltpu.CompilerParams(
                collective_id=0, vmem_limit_bytes=64 * 1024 * 1024, flags=flags,
                disable_bounds_checks=not checks, disable_semaphore_checks=not checks),
        )(x.reshape(512, 512), Wq, Kt, Vt, Wo)
        return out.reshape(2, 256, 512)

    return fn


_fn = make()


def pallas_dist_sparse_attn_causalblk_htp_bs_b2_sq256_skv256_hq4_dh64_kernel(x, Wq, K_ext, V_ext, Wo):
    return _fn(x, Wq, K_ext, V_ext, Wo)
```

```python
import math

import jax
import jax.numpy as jnp
from jax import lax
from jax.experimental import pallas as pl
from jax.experimental.pallas import tpu as pltpu

F32, BF16, I32 = jnp.float32, jnp.bfloat16, jnp.int32
OWN, LEFT, RIGHT, DIAG = range(4)
WQ, WO = range(2)
SHARD = {"o": OWN, "l": LEFT, "r": RIGHT, "d": DIAG}
PAIRS = ((OWN, 0), (OWN, 1), (LEFT, 0), (RIGHT, 1), (LEFT, 1), (RIGHT, 0), (DIAG, 0), (DIAG, 1))
KV_GROUPS = ((0,), (1,), (2, 3), (4, 5), (6, 7))
TILE_ROWS = {0: (1, 4), 1: (1, 4), 2: (0, 1), 5: (2, 3), 3: (3, 4), 4: (3, 4)}
SCORE_SCALE = 0.125 * math.log2(math.e)

HIGH, MARKS, WIRE_TILES = 16, 22, 45
FIRST_LOADS = (0, 2, 7, 16)
SIGNS = -0x7FFF8000
OVERFLOW = 1 << 16


def words(v):
    return pltpu.bitcast(v.astype(BF16), I32)


def as_bf16(w):
    return pltpu.bitcast(w, BF16)


def shift(v, n):
    if n >= 0:
        return v << n if n else v
    return lax.shift_right_logical(v, jnp.full(v.shape, -n, I32))


def reverse_bits(v):
    for n, mask in ((1, 0x55555555), (2, 0x33333333), (4, 0x0F0F0F0F), (8, 0x00FF00FF), (16, 0xFFFF)):
        v = (shift(v, -n) & mask) | ((v & mask) << n)
    return v


def tiles(p, first, count=1):
    tile = first + p * (WIRE_TILES - 2 * first - count)
    return pl.ds(8 * tile if isinstance(tile, int) else pl.multiple_of(8 * tile, 8), 8 * count)


def low_bytes(w):
    return (w[:8] & 0x00FF00FF) | ((w[8:] & 0x00FF00FF) << 8)


def encode_high(ws):
    peak = jnp.zeros((8, 128), F32)
    for w in ws:
        for half in (w, w << 16):
            peak = jnp.maximum(peak, pltpu.bitcast(half & 0x7F800000, F32))
    lane_peak = jnp.broadcast_to(jnp.max(peak, axis=0, keepdims=True), (8, 128))
    lane_top = shift(pltpu.bitcast(lane_peak, I32), -23)
    lower = (peak < lane_peak).astype(I32)
    top = lane_top - lower
    top = (top << 23) | (top << 7)
    planes = [None] * 6
    marks = end = jnp.zeros((8, 128), I32)
    for i, w in enumerate(ws):
        drop = top - (w & 0x7F807F80)
        fields = [(4 + i // 16, shift(w & SIGNS, -(i % 16)))]
        for q, pos in ((shift(drop, -24), 16), (shift(drop, -8) & 0x7F, 0)):
            big = q > 2
            end = end + jnp.where(big, q - 2, 0)
            marks = marks | (1 << (end & 31))
            fields.append((i // 8, shift(jnp.where(big, 3, q), pos + 2 * (i % 8))))
        for k, field in fields:
            planes[k] = field if planes[k] is None else planes[k] | field
    return planes, (shift(marks, -1), end, lower, lane_top)


def merge_marks(pair0, pair1):
    (marks0, end0, lower0, top0), (marks1, end1, lower1, top1) = pair0, pair1
    fits = end0 + end1 <= 29
    shared = (marks0 << 3) | (lower1 << 2) | (lower0 << 1) | jnp.where(fits, reverse_bits(marks1) | 1, 0)
    spill = jnp.where(fits, 0, marks1)
    count = jnp.where(fits, 0, jnp.where((end0 > 29) | (end1 > 31), 2, 1))
    for n in (4, 2, 1):
        spill = spill | pltpu.roll(spill, n, 0)
        count = count + pltpu.roll(count, n, 0)
    worst = jnp.broadcast_to(jnp.max(count.astype(F32), axis=1, keepdims=True), (8, 128))
    meta = top0 | (top1 << 8) | jnp.where(worst > 1.0, OVERFLOW, 0)
    return shared, jnp.where(lax.broadcasted_iota(I32, (8, 128), 0) == 0, spill, meta)[:2]


def decode_high(p, plane, shared, spill, meta):
    top = (shift(meta, -8 * p) & 0xFF) - (shift(shared, -1 - p) & 1)
    yield jnp.where((top & 1) != 0, 0, 0x00800080)
    top = ((top << 23) | (top << 7)) & 0x7F007F00
    marks = jnp.where((shared & 1) != 0, reverse_bits(shared), spill) if p else shift(shared, -3)
    end = jnp.full((8, 128), 0.5, F32)
    for i in range(32):
        if i % 8 == 0:
            code = plane(i // 8)
            big = code & shift(code, -1) & 0x55555555
            code = code - big
        w = top - (shift(code, 8 - 2 * (i % 8)) & 0x03000300)
        for pos in (16, 0):
            rest = marks & (marks + (shift(big, 31 - pos - 2 * (i % 8)) >> 31))
            new_end = jnp.maximum(end, (marks ^ rest).astype(F32))
            w = w - shift(pltpu.bitcast(new_end, I32) - pltpu.bitcast(end, I32), pos - 15)
            marks, end = rest, new_end
        yield w | (shift(plane(4 + i // 16), i % 16) & SIGNS)


def kernel_body(x_hbm, wq_hbm, k_hbm, v_hbm, wo_hbm, o_ref,
                xf, wqf, wof, kf, vf, head, xw, full, wire, trailer, ctx, acc,
                load_sem, send_sem, recv_sem, plain_sem, ready):
    me = lax.axis_index("i")
    right, left = lax.rem(me + 1, 4), lax.rem(me + 3, 4)
    owner = (me, left, right, lax.rem(me + 2, 4))
    odd = lax.rem(me, 2)

    urgent = (me == 1).astype(I32)

    def load_wq(slot, p, first, last, sem):
        rows = pl.ds(32 * first, 32 * (last - first))
        return pltpu.make_async_copy(
            wq_hbm.at[rows, pl.ds(pl.multiple_of(128 * p, 128), 128)], wqf.at[slot, rows], load_sem.at[sem])

    ld_wq = [load_wq(0, urgent, FIRST_LOADS[i], FIRST_LOADS[i + 1], i) for i in range(3)]
    ld_wq_other = load_wq(1, 1 - urgent, 0, 16, 3)
    ld_wo = pltpu.make_async_copy(wo_hbm, wof, load_sem.at[4])
    ld_x = pltpu.make_async_copy(x_hbm, xf, load_sem.at[5])
    ld_kv = [[pltpu.make_async_copy(
        src.at[pl.ds(2 * me, 2), pl.ds(256 * owner[PAIRS[i][0]] + 128 * PAIRS[i][1], 128)],
        dst.at[i], load_sem.at[6 + g]) for i in group for src, dst in ((k_hbm, kf), (v_hbm, vf))]
        for g, group in enumerate(KV_GROUPS)]

    def wait_kv(g):
        for copy in ld_kv[g]:
            copy.wait()

    def remote(src, dst, ssem, rsem, k):
        return pltpu.make_async_remote_copy(
            src, dst, ssem, rsem, device_id=((right, left)[k],), device_id_type=pl.DeviceIdType.MESH)

    def link(k):
        near, a, b = (LEFT, RIGHT)[k], k, 1 - k
        table = {}

        def add(name, src, dst):
            table[name] = remote(src, dst, send_sem.at[k, len(table)], recv_sem.at[k, len(table)], k)

        def part(name, s, d, m, rows):
            add(name, wire.at[s, m, rows], wire.at[d, m, rows])

        for i in range(3):
            part(f"qa{i}", OWN, near, WQ, tiles(a, FIRST_LOADS[i], min(FIRST_LOADS[i + 1], 15) - FIRST_LOADS[i]))
        part("qa3", OWN, near, WQ, tiles(a, 15, 8))
        add("head", wq_hbm.at[pl.ds(480, 32), pl.ds(128 * a, 128)], head.at[k])
        part("qah", OWN, near, WQ, tiles(a, HIGH, 7))
        part("qb0", OWN, near, WQ, tiles(b, 0, FIRST_LOADS[2]))
        part("qb1", OWN, near, WQ, tiles(b, FIRST_LOADS[2], MARKS - FIRST_LOADS[2]))
        part("oah", OWN, near, WO, tiles(a, HIGH, 7))
        part("obh", OWN, near, WO, tiles(b, HIGH, 6))
        for i in range(2):
            add(("qt", "ot")[i], trailer.at[OWN, i], trailer.at[near, i])
            part(f"oa{i}", OWN, near, WO, tiles(a, 8 * i, 8))
            part(f"ob{i}", OWN, near, WO, tiles(b, 8 * i, 8))
        part("fq", near, DIAG, WQ, tiles(a, 0, MARKS + 1 - k))
        part("foh", near, DIAG, WO, tiles(a, HIGH, 6 + k))
        add(("fqt", "fot")[k], trailer.at[near, k], trailer.at[DIAG, k])
        for n in range(4):
            part(f"fo{n}", near, DIAG, WO, tiles(a, 4 * n, 4))
        return table

    links = (link(0), link(1))

    def each(action, names, when):
        for table, cond in zip(links, when):
            def run():
                for name in names.split():
                    if name in table:
                        action(table[name])
            if cond is True:
                run()
            elif cond is not False:
                pl.when(cond)(run)

    def send(names, when=(True, True)):
        each(lambda copy: copy.start(), names, when)

    def sent(names, when=(True, True)):
        each(lambda copy: copy.wait_send(), names, when)

    def receive(names):
        each(lambda copy: copy.wait_recv(), names, (True, True))

    def put_low(m, p, j, rows):
        w = words(rows)
        full[OWN, m, p, pl.ds(16 * j, 16)] = w
        wire[OWN, m, tiles(p, j)] = low_bytes(w)

    def put_high(m, p):
        planes, stream = encode_high([full[OWN, m, p, pl.ds(8 * i, 8)] for i in range(32)])
        for k, plane in enumerate(planes):
            wire[OWN, m, tiles(p, HIGH + k)] = plane
        return stream

    def put_marks(m, pair0, pair1):
        shared, tail = merge_marks(pair0, pair1)
        wire[OWN, m, tiles(0, MARKS)] = shared
        trailer[OWN, m] = tail

    def overflowed(*shards):
        bits = None
        for n, (s, m) in enumerate(shards):
            bit = shift(trailer[s, m, pl.ds(1, 1)] & OVERFLOW, n)
            bits = bit if bits is None else bits | bit
        bits = bits[0, 0]
        return [(bits & (OVERFLOW << n)) != 0 for n in range(len(shards))]

    def plain(s, d, m, k):
        return remote(full.at[s, m], full.at[d, m], plain_sem.at[m, OWN], plain_sem.at[m, d], k)

    def send_plain(s, d, m, k):
        copy = plain(s, d, m, k)
        copy.start()
        copy.wait_send()

    def receive_plain(m, *shards):
        for s, flag in zip(shards, overflowed(*((s, m) for s in shards))):
            @pl.when(flag)
            def _():
                plain(OWN, s, m, 0).wait_recv()
                if s == LEFT:
                    send_plain(LEFT, DIAG, m, 0)

    low_masks, decoders, pending = {}, {}, []

    def add_low(s, m, p, j, high):
        keep, borrow = low_masks[s, m, p]
        v = wire[s, m, tiles(p, j)]
        return [h + low - ((low & borrow) << 1) for h, low in zip(high, (v & keep, shift(v, -8) & keep))]

    def decoder(s, m, p):
        spill, meta = (jnp.broadcast_to(trailer[s, m, pl.ds(r, 1)], (8, 128)) for r in range(2))
        is_plain = (meta & OVERFLOW) != 0
        high = decode_high(p, lambda k: wire[s, m, tiles(p, HIGH + k)], wire[s, m, tiles(0, MARKS)], spill, meta)
        low_masks[s, m, p] = (jnp.where(is_plain, 0, 0x00FF00FF), next(high))
        for g in range(4):
            out = [jnp.where(is_plain, full[s, m, p, pl.ds(64 * g + 8 * i, 8)], next(high)) for i in range(8)]
            if m == WQ:
                out = [w for j in range(4) for w in add_low(s, m, p, 4 * g + j, out[2 * j:2 * j + 2])]
            full[s, m, p, pl.ds(64 * g, 64)] = jnp.concatenate(out, axis=0)
            pending.append(out[-1])
            yield

    def after_decoding(v):
        if not pending:
            return v
        first = v[:8]
        while pending:
            w = pending.pop()
            first = jnp.where(me < 0, w if v.dtype == I32 else pltpu.bitcast(w, v.dtype), first)
        return jnp.concatenate([first, v[8:]], axis=0)

    def kv_tiles(ref):
        lo = lax.broadcasted_iota(I32, (64, 128), 1) < 64
        zero = jnp.zeros((64, 128), F32)
        out = []
        for j in range(2):
            t = after_decoding(ref[:, pl.ds(128 * j, 128)])
            a, b = t[:64], t[64:]
            both = (jnp.where(lo, a, 0.0), jnp.where(lo, 0.0, pltpu.roll(b, 64, 1)))
            out += [jnp.concatenate(part, axis=0).astype(BF16) for part in ((a, zero), (zero, b), both)]
        return out

    def per_head(x, r, op, across, identity):
        lo = lax.broadcasted_iota(I32, (64, 128), 1) < 64
        a = [x[r, t] if t % 3 == 0 else jnp.where(lo, x[r, t], identity) for t in (0, 2, 3, 5) if (r, t) in x]
        b = [x[r, t] if t % 3 == 1 else jnp.where(lo, identity, x[r, t]) for t in (1, 2, 4, 5) if (r, t) in x]
        a, b = (across(v[0] if len(v) == 1 else op(*v), axis=1, keepdims=True) for v in (a, b))
        return a, b, jnp.where(lo, a, b)

    state = {}

    def attend(stage, u):
        i, b = divmod(u, 2)
        s, p = PAIRS[i]
        if stage == "Q":
            state[u] = jnp.dot(as_bf16(xw[pl.ds(128 * b, 128), :]), as_bf16(after_decoding(full[s, WQ, p])),
                               preferred_element_type=F32)
        elif stage == "S":
            q, kt, scores = state[u], kv_tiles(kf.at[i, b]), {}
            for t, (r0, r1) in TILE_ROWS.items():
                v = jnp.dot(q[64 * r0:64 * r1].astype(BF16), kt[t], preferred_element_type=F32)
                for r in range(r0, r1):
                    scores[r, t] = v[64 * (r - r0):64 * (r - r0 + 1)]
            state[u] = scores
        elif stage == "E":
            scores, weights = state[u], {}
            for r in range(4):
                row_max = per_head(scores, r, jnp.maximum, jnp.max, -jnp.inf)
                for t in range(6):
                    if (r, t) in scores:
                        weights[r, t] = jnp.exp2(scores[r, t] - row_max[t % 3])
            state[u] = weights, [per_head(weights, r, jnp.add, jnp.sum, 0.0)[2] for r in range(4)]
        else:
            (weights, total), vt, out = state[u], kv_tiles(vf.at[i, b]), {}
            for t, (r0, r1) in TILE_ROWS.items():
                w = jnp.concatenate([weights[r, t] for r in range(r0, r1)], axis=0).astype(BF16)
                v = lax.dot_general(w, vt[t], (((1,), (1,)), ((), ())), preferred_element_type=F32)
                for r in range(r0, r1):
                    part = v[64 * (r - r0):64 * (r - r0 + 1)]
                    out[r] = out[r] + part if r in out else part
            for r in range(4):
                inv = pltpu.reciprocal(total[r], approx=True)
                inv = inv * (2.0 - total[r] * inv)
                ctx[s, p, pl.ds(128 * b + 32 * r, 32)] = words(out[r] * inv)

    def project(n, terms):
        ws = []
        for s, p in terms:
            w = full[s, WO, p, pl.ds(64 * n, 64)]
            if s != OWN:
                w = jnp.concatenate([t for j in range(4) for t in add_low(
                    s, WO, p, 4 * n + j, (w[16 * j:16 * j + 8], w[16 * j + 8:16 * j + 16]))], axis=0)
            ws.append(as_bf16(after_decoding(w)))
        rows = 128 * len(terms)
        for r0 in range(0, 512, rows):
            total = None if terms[0] == (OWN, 0) else acc[n, pl.ds(r0, rows)]
            for (s, p), w in zip(terms, ws):
                t = jnp.dot(as_bf16(ctx[s, p, pl.ds(r0 // 2, rows // 2)]), w, preferred_element_type=F32)
                total = t if total is None else total + t
            if terms[0][0] == DIAG:
                o_ref[pl.ds(r0, rows), pl.ds(128 * n, 128)] = total.astype(o_ref.dtype)
            else:
                acc[n, pl.ds(r0, rows)] = total

    def compute(steps):
        for step in steps.split():
            if step[0] in "WH":
                key = (SHARD[step[1]], WQ if step[0] == "W" else WO, int(step[2]))
                next(decoders.setdefault(key, decoder(*key)))
            elif step[0] == "M":
                project(int(step[1]), [(SHARD[t[0]], int(t[1])) for t in step[3:].split(",")])
            else:
                attend(step[0], int(step[1:]))
        pending.clear()

    def signal_neighbours(sem):
        for chip in (right, left):
            pl.semaphore_signal(sem, inc=1, device_id=(chip,), device_id_type=pl.DeviceIdType.MESH)

    barrier = pltpu.get_barrier_semaphore()
    into_0, not_into_0 = (me == 3, me == 1), (me != 3, me != 1)
    ld_wq[0].start()
    pl.when(me != 2)(lambda: signal_neighbours(barrier))
    pl.when(me != 0)(lambda: pl.semaphore_wait(barrier, 2 - odd))
    send("head", into_0)
    pl.when(me == 2)(lambda: signal_neighbours(ready))
    ld_wq[1].start()
    ld_wq[2].start()
    for i in range(3):
        ld_wq[i].wait()
        for j in range(FIRST_LOADS[i], FIRST_LOADS[i + 1]):
            put_low(WQ, urgent, j, wqf[0, pl.ds(32 * j, 32)])
        send(f"qa{i}", (me >= 2, me == 1))
        if i == 0:
            for copy in [ld_wq_other, ld_wo, ld_x] + [copy for group in ld_kv for copy in group]:
                copy.start()
        if i == 1:
            send("qb0", (False, me == 2))
    early = put_high(WQ, urgent)
    ld_wq_other.wait()
    for j in range(16):
        put_low(WQ, 1 - urgent, j, wqf[1, pl.ds(32 * j, 32)])
    send("qa0 qa1 qa2", (False, me == 2))
    late = put_high(WQ, 1 - urgent)
    put_marks(WQ, [jnp.where(me == 1, b, a) for a, b in zip(early, late)],
              [jnp.where(me == 1, a, b) for a, b in zip(early, late)])
    pl.when(me == 0)(lambda: pl.semaphore_wait(barrier, 2))
    pl.when(odd == 1)(lambda: pl.semaphore_wait(ready, 1))
    send("qa0 qa1 qa2", (me <= 1, (me == 0) | (me == 3)))
    send("qah", into_0)
    send("qa3", not_into_0)
    send("qt")
    send("qb0", (True, me != 2))
    send("qb1")

    ld_wo.wait()
    for p in range(2):
        for j in range(16):
            put_low(WO, p, j, wof[pl.ds(128 * p + 32 * (j % 4), 32), pl.ds(128 * (j // 4), 128)])
    put_marks(WO, put_high(WO, 0), put_high(WO, 1))
    for m, flag in enumerate(overflowed((OWN, WQ), (OWN, WO))):
        @pl.when(flag)
        def _():
            send_plain(OWN, LEFT, m, 0)
            send_plain(OWN, RIGHT, m, 1)
    send("oah ot oa0")

    ld_x.wait()
    xw[...] = words(xf[...] * SCORE_SCALE)
    compute("Q1 Q0")

    sent("qa0 qa1 qa2")
    wait_kv(0)
    compute("Q3 S0 Q2 S1 E1 E0 P0 P1")

    receive("qa0 qa1 qa2 qt")
    pl.when(me != 0)(lambda: receive("qa3"))

    @pl.when(me == 0)
    def _():
        receive("head qah")
        for k in range(2):
            wire[(LEFT, RIGHT)[k], WQ, tiles(k, 15)] = low_bytes(words(head[k]))

    send("fq fqt oa1 obh")
    receive_plain(WQ, LEFT, RIGHT)
    wait_kv(1)
    compute("M2:o0 Wl0 M1:o0 Wl0 S3 Wl0 E3 Wl0 S2 Wr1 M3:o0 Wr1 E2 M0:o0 Wr1 P2 Q4 Wr1 P3 Q5")

    wait_kv(2)
    compute("S4 Q6 S6 Q7 S5 E5 E4 E6 P4 P6 S7 P5 E7 P7")

    receive("qb0 qb1 oah ot")
    send("foh fot ob0 ob1")
    receive_plain(WO, LEFT, RIGHT)
    wait_kv(3)
    compute("M1:o1 Wl1 M0:o1 Wl1 M2:o1 Wl1 Wl1 M3:o1 Q8 Wr0 Wr0 Wr0 S8 Hl0 Q9 Wr0 Q10 Hl0 S9 Hr1 Q11 "
            "Hl0 Hl0 Hr1 E8 S10 Hr1 P8 Hr1 S11 E9 E10 P9 E11 P10 P11")

    def pass_on_last():
        receive("oa1")
        send("fo2 fo3")

    receive("oa0")
    send("fo0 fo1")
    sent("head qah", into_0)
    sent("qa3", not_into_0)
    sent("qt qb0 qb1 oah ot oa0")
    pl.when(me != 0)(pass_on_last)
    receive("fq fqt")
    receive_plain(WQ, DIAG)
    wait_kv(4)
    compute("M1:l0,r1 Wd0 Wd0 M0:l0,r1 Wd0 Wd0 Q12 Wd1 S12 Wd1 Q13 Wd1 Wd1 Q14 S13 Q15 E12 S14 E13 "
            "P13 P12 E14 S15 E15 P14 P15")

    pl.when(me == 0)(pass_on_last)
    receive("obh")
    compute("M2:l0 Hl1 Hl1 M3:l0 M2:r1 Hr0 M3:r1 Hr0 Hl1 Hr0 Hr0 Hl1")

    receive("foh fot ob0")
    receive_plain(WO, DIAG)
    compute("M0:r0 M1:l1 M0:l1 Hd1 M1:r0 Hd0 Hd0 Hd0 Hd1 Hd1 Hd1 Hd0")

    @pl.when(me != 0)
    def _():
        receive("ob1 fo0 fo1")
        compute("M2:l1,r0 M3:l1,r0 M0:d0,d1 M1:d0,d1")
        sent("fq fqt oa1 obh foh fot ob0 ob1 fo0 fo1 fo2 fo3")
        receive("fo2 fo3")
        compute("M2:d0,d1 M3:d0,d1")

    @pl.when(me == 0)
    def _():
        receive("ob1")
        compute("M2:l1,r0 M3:l1,r0")
        for n, done in enumerate(("fq fqt oa1", "obh foh fot ob0", "ob1 fo0 fo1", "fo2 fo3")):
            sent(done)
            receive(f"fo{n}")
            compute(f"M{n}:d0,d1")


def pallas_dist_sparse_attn_causalblk_htp_bs_b2_sq256_skv256_hq4_dh64_kernel(
    x: jax.Array,
    Wq: jax.Array,
    K_ext: jax.Array,
    V_ext: jax.Array,
    Wo: jax.Array,
):
    Kt = jnp.transpose(K_ext, (0, 2, 3, 1)).reshape(8, 1024, 256)
    Vt = jnp.transpose(V_ext, (0, 2, 3, 1)).reshape(8, 1024, 256)
    out = pl.pallas_call(
        kernel_body,
        out_shape=jax.ShapeDtypeStruct((512, 512), BF16),
        in_specs=[pl.BlockSpec(memory_space=pl.ANY)] * 5,
        out_specs=pl.BlockSpec(memory_space=pltpu.VMEM),
        scratch_shapes=[
            pltpu.VMEM((512, 512), F32),
            pltpu.VMEM((2, 512, 128), F32),
            pltpu.VMEM((256, 512), F32),
            pltpu.VMEM((8, 2, 128, 256), F32),
            pltpu.VMEM((8, 2, 128, 256), F32),
            pltpu.VMEM((2, 32, 128), F32),
            pltpu.VMEM((256, 512), I32),
            pltpu.VMEM((4, 2, 2, 256, 128), I32),
            pltpu.VMEM((4, 2, 8 * WIRE_TILES, 128), I32),
            pltpu.VMEM((4, 2, 2, 128), I32),
            pltpu.VMEM((4, 2, 256, 128), I32),
            pltpu.VMEM((4, 512, 128), F32),
            pltpu.SemaphoreType.DMA((11,)),
            pltpu.SemaphoreType.DMA((2, 23)),
            pltpu.SemaphoreType.DMA((2, 23)),
            pltpu.SemaphoreType.DMA((2, 4)),
            pltpu.SemaphoreType.REGULAR,
        ],
        compiler_params=pltpu.CompilerParams(
            collective_id=0,
            vmem_limit_bytes=64 * 1024 * 1024,
            disable_bounds_checks=True,
            disable_semaphore_checks=True,
        ),
    )(x.reshape(512, 512), Wq, Kt, Vt, Wo)
    return out.reshape(2, 256, 512)
```
